```python
import numpy as np

kernel_name = "dist_max_ax1_xy_m4096_n1024"

def setup_inputs():
    return {"x": np.random.randn(8192, 2048).astype(np.float32)}

def reference(x: np.ndarray) -> np.ndarray:
    return np.max(x, axis=1, keepdims=True)
```

```python
import jax
import jax.numpy as jnp
from jax import lax
from jax.experimental import pallas as pl
from jax.experimental.pallas import tpu as pltpu

_MESH = pl.DeviceIdType.MESH
_CHUNKS = (2048, 1024, 512, 256, 128, 128)
_SEND_AFTER = (4, 5)


def pallas_dist_max_ax1_xy_m4096_n1024_kernel(x: jax.Array):
    m, n = x.shape
    chunks = _CHUNKS
    assert sum(chunks) == m and n % 128 == 0
    offs = [sum(chunks[:i]) for i in range(len(chunks))]

    def body(x_hbm, o_ref, buf, part, recv, sems, ssems, rsems):
        nbr = (lax.axis_index("x"), 1 - lax.axis_index("y"))
        cps = []
        for i, (o, c) in enumerate(zip(offs, chunks)):
            cp = pltpu.make_async_copy(
                x_hbm.at[pl.ds(o, c)], buf.at[pl.ds(o, c)], sems.at[i])
            cp.start()
            cps.append(cp)
        bar = pltpu.get_barrier_semaphore()
        pl.semaphore_signal(bar, 1, device_id=nbr, device_id_type=_MESH)
        sent = 0
        rds = []
        for i, (o, c) in enumerate(zip(offs, chunks)):
            cps[i].wait()

            def blk(b, carry, o=o):
                r0 = pl.multiple_of(o + b * 128, 128)
                t = buf[pl.ds(r0, 128), 0:128]
                for j in range(1, n // 128):
                    t = jnp.maximum(t, buf[pl.ds(r0, 128), j * 128:(j + 1) * 128])
                part[:, pl.ds(r0, 128)] = jnp.max(t.T, axis=0, keepdims=True)
                return carry

            if c == 128:
                blk(0, 0)
            else:
                lax.fori_loop(0, c // 128, blk, 0)
            if i in _SEND_AFTER:
                if not rds:
                    pl.semaphore_wait(bar, 1)
                k = len(rds)
                end = o + c
                rd = pltpu.make_async_remote_copy(
                    part.at[:, pl.ds(sent, end - sent)],
                    recv.at[:, pl.ds(sent, end - sent)],
                    ssems.at[k], rsems.at[k], device_id=nbr, device_id_type=_MESH)
                rd.start()
                rds.append((rd, sent, end))
                sent = end
        for rd, a, b in rds:
            rd.wait_recv()
            o_ref[:, a:b] = jnp.maximum(part[:, a:b], recv[:, a:b])
        for rd, a, b in rds:
            rd.wait_send()

    out = pl.pallas_call(
        body,
        out_shape=jax.ShapeDtypeStruct((1, m), x.dtype),
        in_specs=[pl.BlockSpec(memory_space=pl.ANY)],
        out_specs=pl.BlockSpec(memory_space=pltpu.VMEM),
        scratch_shapes=[
            pltpu.VMEM((m, n), x.dtype),
            pltpu.VMEM((1, m), x.dtype),
            pltpu.VMEM((1, m), x.dtype),
            pltpu.SemaphoreType.DMA((len(chunks),)),
            pltpu.SemaphoreType.DMA((len(_SEND_AFTER),)),
            pltpu.SemaphoreType.DMA((len(_SEND_AFTER),)),
        ],
        compiler_params=pltpu.CompilerParams(
            vmem_limit_bytes=64 * 1024 * 1024, collective_id=0),
    )(x)
    return out.reshape(m, 1)
```

```python
import jax
import jax.numpy as jnp
from jax import lax
from jax.experimental import pallas as pl
from jax.experimental.pallas import tpu as pltpu

_MESH = pl.DeviceIdType.MESH
_B = 128
_MAIN = (1792, 1024, 512, 256, 128, 128)
_TAIL = (64, 32, 32)
_SENDS = (2, 5)
_RAW = ((64, -1), (64, 0))
_RAW_AT = 3


def pallas_dist_max_ax1_xy_m4096_n1024_kernel(x: jax.Array):
    m, n = x.shape
    b = _B
    s0 = 2 * b
    assert sum(_MAIN) == m - s0 and sum(_TAIL) == b and n % 128 == 0
    offs = [s0 + sum(_MAIN[:i]) for i in range(len(_MAIN))]
    toffs = [sum(_TAIL[:i]) for i in range(len(_TAIL))]
    nloc = len(_MAIN) + len(_TAIL)
    nsend = len(_RAW) + len(_SENDS) + 1

    def colmax(ref, r0, rows):
        cols = [ref[pl.ds(r0, rows), j * 128:(j + 1) * 128] for j in range(n // 128)]
        while len(cols) > 1:
            nxt = [jnp.maximum(cols[i], cols[i + 1]) for i in range(0, len(cols) - 1, 2)]
            cols = nxt + cols[len(nxt) * 2:]
        return cols[0]

    def body(x_hbm, o_ref, buf, tbuf, rbuf, part, recv):
        def scoped(sems, ssems, rsem_raw, rsem_part, rsem_fin):
            cps = []
            for i, (o, c) in enumerate(zip(offs, _MAIN)):
                cp = pltpu.make_async_copy(
                    x_hbm.at[pl.ds(o, c)], buf.at[pl.ds(o - s0, c)], sems.at[i])
                if i == 0:
                    cp.start()
                cps.append(cp)
            my = lax.axis_index("y")
            nbr = (lax.axis_index("x"), 1 - my)
            own0 = pl.multiple_of(my * b, b)
            oth0 = pl.multiple_of((1 - my) * b, b)
            bar = pltpu.get_barrier_semaphore()
            pl.semaphore_signal(bar, 1, device_id=nbr, device_id_type=_MESH)
            for cp in cps[1:]:
                cp.start()
            tcps = []
            for i, (o, c) in enumerate(zip(toffs, _TAIL)):
                cp = pltpu.make_async_copy(
                    x_hbm.at[pl.ds(pl.multiple_of(own0 + o, 8), c)],
                    tbuf.at[pl.ds(o, c)], sems.at[len(_MAIN) + i])
                cp.start()
                tcps.append(cp)
            pl.semaphore_wait(bar, 1)
            started = []

            def remote(src, dst, rsem):
                rd = pltpu.make_async_remote_copy(
                    src, dst, ssems.at[len(started)], rsem,
                    device_id=nbr, device_id_type=_MESH)
                rd.start()
                started.append(rd)

            def raw_send(after):
                o = 0
                for r, a in _RAW:
                    if a == after:
                        remote(x_hbm.at[pl.ds(pl.multiple_of(oth0 + o, 8), r)],
                               rbuf.at[pl.ds(o, r)], rsem_raw)
                    o += r

            raw_send(-1)
            sent = 0
            acc = None
            for i, (o, c) in enumerate(zip(offs, _MAIN)):
                cps[i].wait()
                raw_send(i)

                def blk(k, carry, o=o):
                    r0 = pl.multiple_of(o - s0 + k * b, b)
                    part[:, pl.ds(r0, b)] = jnp.max(
                        colmax(buf, r0, b).T, axis=0, keepdims=True)
                    return carry

                if c == b:
                    blk(0, 0)
                else:
                    lax.fori_loop(0, c // b, blk, 0)
                if i in _SENDS:
                    end = o - s0 + c
                    remote(part.at[:, pl.ds(sent, end - sent)],
                           recv.at[:, pl.ds(sent, end - sent)], rsem_part)
                    sent = end
                if i == _RAW_AT:
                    pltpu.make_async_copy(rbuf, rbuf, rsem_raw).wait()
                    acc = jnp.broadcast_to(
                        jnp.max(colmax(rbuf, 0, b).T, axis=0, keepdims=True), (8, b))
            diag = (lax.broadcasted_iota(jnp.int32, (8, b), 1)
                    - lax.broadcasted_iota(jnp.int32, (8, b), 0))
            for i, (o, c) in enumerate(zip(toffs, _TAIL)):
                tcps[i].wait()
                mx = jnp.max(colmax(tbuf, o, c), axis=1, keepdims=True)
                for k in range(c // 8):
                    mk = jnp.broadcast_to(mx[8 * k:8 * k + 8], (8, b))
                    acc = jnp.where(diag == o + 8 * k, mk, acc)
            o_ref[:, pl.ds(own0, b)] = jnp.max(acc, axis=0, keepdims=True)
            remote(o_ref.at[:, pl.ds(own0, b)], o_ref.at[:, pl.ds(own0, b)], rsem_fin)
            pltpu.make_async_copy(recv, recv, rsem_part).wait()
            o_ref[:, s0:] = jnp.maximum(part[...], recv[...])
            for rd in started:
                rd.wait_send()
            pltpu.make_async_copy(
                o_ref.at[:, pl.ds(oth0, b)], o_ref.at[:, pl.ds(oth0, b)], rsem_fin).wait()

        pl.run_scoped(
            scoped,
            pltpu.SemaphoreType.DMA((nloc,)),
            pltpu.SemaphoreType.DMA((nsend,)),
            pltpu.SemaphoreType.DMA,
            pltpu.SemaphoreType.DMA,
            pltpu.SemaphoreType.DMA,
        )

    out = pl.pallas_call(
        body,
        out_shape=jax.ShapeDtypeStruct((1, m), x.dtype),
        in_specs=[pl.BlockSpec(memory_space=pl.ANY)],
        out_specs=pl.BlockSpec(memory_space=pltpu.VMEM),
        scratch_shapes=[
            pltpu.VMEM((m - s0, n), x.dtype),
            pltpu.VMEM((b, n), x.dtype),
            pltpu.VMEM((b, n), x.dtype),
            pltpu.VMEM((1, m - s0), x.dtype),
            pltpu.VMEM((1, m - s0), x.dtype),
        ],
        compiler_params=pltpu.CompilerParams(
            vmem_limit_bytes=64 * 1024 * 1024, collective_id=0),
    )(x)
    return out.reshape(m, 1)
```

```python
import jax
import jax.numpy as jnp
from jax import lax
from jax.experimental import pallas as pl
from jax.experimental.pallas import tpu as pltpu

_MESH = pl.DeviceIdType.MESH
_B = 128
_X = 192
_S = 104
_Q = 72
_MAIN = (1536, 1024, 384, 128, 128, 128)
_TAIL = (64, 32, 32)
_SENDS = (1, 5)
_BOUNCE_AT, _X_AT, _ZONE_AT, _OWN_AT = 0, 2, 3, 4
_UNROLL = 2


def _cdiv(a, b):
    return -(-a // b)


def pallas_dist_max_ax1_xy_m4096_n1024_kernel(x: jax.Array):
    m, n = x.shape
    dt = x.dtype
    b, nx, ns, nq = _B, _X, _S, _Q
    zrows = _cdiv(nx + ns + 2 * nq, b) * b
    nzl = zrows - nx - ns - 2 * nq
    z0 = 2 * b
    s0 = z0 + zrows
    nzb = zrows // b
    nxb = _cdiv(nx, b)
    pb0 = nx // b
    p0 = z0 + pb0 * b
    pz = s0 - p0
    yq = nx + ns + nzl
    assert sum(_MAIN) == m - s0 and sum(_TAIL) == b and n % 128 == 0 and nzl > 0
    assert _X_AT <= _ZONE_AT and _SENDS[-1] == len(_MAIN) - 1
    offs = [s0 + sum(_MAIN[:i]) for i in range(len(_MAIN))]
    toffs = [sum(_TAIL[:i]) for i in range(len(_TAIL))]
    nm = len(_MAIN)
    nloc = nm + len(_TAIL) + 4
    nsend = 7 + len(_SENDS)
    r_q, r_own, r_x, r_part, r_xa, r_xb, r_fin = range(7)

    def body(x_hbm, o_ref, buf, zs, zl, zq, tbuf, rq, rown, rx, part, recv,
             hx, xa, xb, sm):
        diag = (lax.broadcasted_iota(jnp.int32, (8, b), 1)
                - lax.broadcasted_iota(jnp.int32, (8, b), 0))

        def colmax(ref, r0, rows):
            cols = [ref[pl.ds(r0, rows), j * 128:(j + 1) * 128]
                    for j in range(n // 128)]
            while len(cols) > 1:
                nxt = [jnp.maximum(cols[i], cols[i + 1])
                       for i in range(0, len(cols) - 1, 2)]
                cols = nxt + cols[2 * len(nxt):]
            return cols[0]

        def place(t, g0, lo, hi, accs):
            mx = jnp.max(t, axis=1, keepdims=True)
            for k in range(t.shape[0] // 8):
                mk = jnp.broadcast_to(mx[8 * k:8 * k + 8], (8, b))
                for j in range((lo + 8 * k) // b, (hi + 8 * k) // b + 1):
                    accs[j] = jnp.where(diag == g0 + 8 * k - j * b, mk, accs[j])

        def empty(k):
            return [jnp.full((8, b), -jnp.inf, dt) for _ in range(k)]

        def fold(acc):
            return jnp.max(acc, axis=0, keepdims=True)

        def block_max(ref, r0):
            accs = empty(1)
            place(colmax(ref, r0, b), 0, 0, 0, accs)
            return fold(accs[0])

        def scoped(sems, ssems, rsems, reply):
            e = nm + len(_TAIL)
            cps = [pltpu.make_async_copy(x_hbm.at[pl.ds(o, c)],
                                         buf.at[pl.ds(o - s0, c)], sems.at[i])
                   for i, (o, c) in enumerate(zip(offs, _MAIN))]
            cps[0].start()
            s_in = pltpu.make_async_copy(x_hbm.at[pl.ds(z0 + nx, ns)], sm, sems.at[e])
            s_in.start()
            s_out = pltpu.make_async_copy(sm, zs, sems.at[e + 1])

            cx, cy = lax.axis_index("x"), lax.axis_index("y")
            ynbr, xnbr, dnbr = (cx, 1 - cy), (1 - cx, cy), (1 - cx, 1 - cy)
            odd = (cx + cy) % 2 == 1
            succ = (jnp.where(odd, 1 - cx, cx), jnp.where(odd, cy, 1 - cy))
            pred = (jnp.where(odd, cx, 1 - cx), jnp.where(odd, 1 - cy, cy))
            bar = pltpu.get_barrier_semaphore()
            pl.semaphore_signal(bar, 1, device_id=succ, device_id_type=_MESH)

            own0 = pl.multiple_of(cy * b, b)
            oth0 = pl.multiple_of((1 - cy) * b, b)
            qk = pl.multiple_of(yq + cy * nq, 8)
            qo = pl.multiple_of(yq + (1 - cy) * nq, 8)
            zcps = [
                pltpu.make_async_copy(x_hbm.at[pl.ds(z0 + nx + ns, nzl)], zl,
                                      sems.at[e + 2]),
                pltpu.make_async_copy(x_hbm.at[pl.ds(pl.multiple_of(z0 + qk, 8), nq)],
                                      zq, sems.at[e + 3]),
            ]
            tcps = [pltpu.make_async_copy(
                        x_hbm.at[pl.ds(pl.multiple_of(own0 + o, 8), c)],
                        tbuf.at[pl.ds(o, c)], sems.at[nm + i])
                    for i, (o, c) in enumerate(zip(toffs, _TAIL))]
            for cp in zcps + cps[1:] + tcps:
                cp.start()

            sends = []

            def remote(src, dst, r, dev):
                rd = pltpu.make_async_remote_copy(
                    src, dst, ssems.at[len(sends)], rsems.at[r],
                    device_id=dev, device_id_type=_MESH)
                sends.append(rd)
                return rd

            raw_q = remote(x_hbm.at[pl.ds(pl.multiple_of(z0 + qo, 8), nq)], rq, r_q, ynbr)
            raw_own = remote(x_hbm.at[pl.ds(oth0, b)], rown, r_own, ynbr)
            raw_x = remote(x_hbm.at[pl.ds(z0, nx)], rx, r_x, xnbr)

            pl.semaphore_wait(bar, 1)
            pl.semaphore_signal(reply, 1, device_id=pred, device_id_type=_MESH)

            @pl.when(odd)
            def _():
                raw_q.start()
                raw_own.start()
                pl.semaphore_wait(reply, 1)
                raw_x.start()

            @pl.when(jnp.logical_not(odd))
            def _():
                raw_x.start()
                pl.semaphore_wait(reply, 1)
                raw_q.start()
                raw_own.start()

            sent = pz
            acc = None
            for i, (o, c) in enumerate(zip(offs, _MAIN)):
                cps[i].wait()
                if i == _BOUNCE_AT:
                    s_in.wait()
                    s_out.start()
                if i == _X_AT:
                    raw_q.wait_recv()
                    raw_x.wait_recv()
                    accs = empty(nxb)
                    place(colmax(rx, 0, nx), 0, 0, 0, accs)
                    for j in range(nxb):
                        hx[:, j * b:(j + 1) * b] = fold(accs[j])
                    remote(hx, xb, r_xb, dnbr).start()
                    remote(hx, xa, r_xa, xnbr).start()

                nb = c // b
                u = max(d for d in range(1, _UNROLL + 1) if nb % d == 0)

                def blocks(k, carry, o=o, u=u):
                    for j in range(u):
                        r0 = pl.multiple_of(o - s0 + (k * u + j) * b, b)
                        part[:, pl.ds(pl.multiple_of(r0 + pz, b), b)] = block_max(buf, r0)
                    return carry

                if nb == u:
                    blocks(0, 0)
                else:
                    lax.fori_loop(0, nb // u, blocks, 0)
                if i in _SENDS:
                    done = o + c - p0
                    remote(part.at[:, pl.ds(sent, done - sent)],
                           recv.at[:, pl.ds(sent, done - sent)], r_part, ynbr).start()
                    sent = done
                if i == _ZONE_AT:
                    for cp in zcps:
                        cp.wait()
                    s_out.wait()
                    accs = empty(nzb)
                    place(jnp.maximum(colmax(zq, 0, nq), colmax(rq, 0, nq)),
                          qk, yq, yq + nq, accs)
                    place(colmax(zl, 0, nzl), nx + ns, nx + ns, nx + ns, accs)
                    place(colmax(zs, 0, ns), nx, nx, nx, accs)
                    for j in range(pb0, nzb):
                        part[:, (j - pb0) * b:(j - pb0 + 1) * b] = fold(accs[j])
                    remote(part.at[:, pl.ds(0, pz)], recv.at[:, pl.ds(0, pz)],
                           r_part, ynbr).start()
                if i == _OWN_AT:
                    raw_own.wait_recv()
                    acc = [jnp.broadcast_to(block_max(rown, 0), (8, b))]

            for i, (o, c) in enumerate(zip(toffs, _TAIL)):
                tcps[i].wait()
                place(colmax(tbuf, o, c), o, o, o, acc)
            o_ref[:, pl.ds(own0, b)] = fold(acc[0])
            remote(o_ref.at[:, pl.ds(own0, b)], o_ref.at[:, pl.ds(own0, b)],
                   r_fin, ynbr).start()

            pltpu.make_async_copy(xa, xa, rsems.at[r_xa]).wait()
            pltpu.make_async_copy(xb, xb, rsems.at[r_xb]).wait()
            pltpu.make_async_copy(recv, recv, rsems.at[r_part]).wait()
            ov = (nxb - pb0) * b
            if pb0:
                o_ref[:, z0:p0] = jnp.maximum(xa[:, :pb0 * b], xb[:, :pb0 * b])
            if ov:
                o_ref[:, p0:p0 + ov] = jnp.maximum(
                    jnp.maximum(xa[:, pb0 * b:], xb[:, pb0 * b:]),
                    jnp.maximum(part[:, :ov], recv[:, :ov]))
            o_ref[:, p0 + ov:] = jnp.maximum(part[:, ov:], recv[:, ov:])
            assert len(sends) == nsend
            for rd in sends:
                rd.wait_send()
            pltpu.make_async_copy(o_ref.at[:, pl.ds(oth0, b)],
                                  o_ref.at[:, pl.ds(oth0, b)], rsems.at[r_fin]).wait()

        pl.run_scoped(
            scoped,
            pltpu.SemaphoreType.DMA((nloc,)),
            pltpu.SemaphoreType.DMA((nsend,)),
            pltpu.SemaphoreType.DMA((7,)),
            pltpu.SemaphoreType.REGULAR,
        )

    out = pl.pallas_call(
        body,
        out_shape=jax.ShapeDtypeStruct((1, m), dt),
        in_specs=[pl.BlockSpec(memory_space=pl.ANY)],
        out_specs=pl.BlockSpec(memory_space=pltpu.VMEM),
        scratch_shapes=[
            pltpu.VMEM((m - s0, n), dt),
            pltpu.VMEM((ns, n), dt),
            pltpu.VMEM((nzl, n), dt),
            pltpu.VMEM((nq, n), dt),
            pltpu.VMEM((b, n), dt),
            pltpu.VMEM((nq, n), dt),
            pltpu.VMEM((b, n), dt),
            pltpu.VMEM((nx, n), dt),
            pltpu.VMEM((1, m - p0), dt),
            pltpu.VMEM((1, m - p0), dt),
            pltpu.VMEM((1, nxb * b), dt),
            pltpu.VMEM((1, nxb * b), dt),
            pltpu.VMEM((1, nxb * b), dt),
            pltpu.SMEM((ns, n), dt),
        ],
        compiler_params=pltpu.CompilerParams(
            vmem_limit_bytes=64 * 1024 * 1024, collective_id=0),
    )(x)
    return out.reshape(m, 1)
```

```python
import jax
import jax.numpy as jnp
from jax import lax
from jax.experimental import pallas as pl
from jax.experimental.pallas import tpu as pltpu

_MESH = pl.DeviceIdType.MESH
_B = 128
_X = 192
_S = 104
_Q = 72
_MAIN = (1536, 1024, 384, 128, 128, 128)
_TAIL = (64, 32, 32)
_SENDS = (1, 5)
_BOUNCE_AT, _X_AT, _ZONE_AT, _OWN_AT = 0, 2, 3, 4
_UNROLL = 2


def _cdiv(a, b):
    return -(-a // b)


def pallas_dist_max_ax1_xy_m4096_n1024_kernel(x: jax.Array):
    m, n = x.shape
    dt = x.dtype
    b, nx, ns, nq = _B, _X, _S, _Q
    zrows = _cdiv(nx + ns + 2 * nq, b) * b
    nzl = zrows - nx - ns - 2 * nq
    z0 = 2 * b
    s0 = z0 + zrows
    nzb = zrows // b
    nxb = _cdiv(nx, b)
    pb0 = nx // b
    p0 = z0 + pb0 * b
    pz = s0 - p0
    yq = nx + ns + nzl
    assert sum(_MAIN) == m - s0 and sum(_TAIL) == b and n % 128 == 0 and nzl > 0
    assert _SENDS[-1] == len(_MAIN) - 1
    offs = [s0 + sum(_MAIN[:i]) for i in range(len(_MAIN))]
    toffs = [sum(_TAIL[:i]) for i in range(len(_TAIL))]
    nm = len(_MAIN)
    nloc = nm + len(_TAIL) + 4
    nsend = 7 + len(_SENDS)
    r_q, r_own, r_x, r_part, r_xa, r_fin = range(6)

    def body(x_hbm, o_ref, buf, zs, zl, zq, tbuf, rq, rown, rx, part, recv,
             hx, xa, xb, sm, xb_sem):
        diag = (lax.broadcasted_iota(jnp.int32, (8, b), 1)
                - lax.broadcasted_iota(jnp.int32, (8, b), 0))

        def colmax(ref, r0, rows):
            cols = [ref[pl.ds(r0, rows), j * 128:(j + 1) * 128]
                    for j in range(n // 128)]
            while len(cols) > 1:
                nxt = [jnp.maximum(cols[i], cols[i + 1])
                       for i in range(0, len(cols) - 1, 2)]
                cols = nxt + cols[2 * len(nxt):]
            return cols[0]

        def place(t, g0, lo, hi, accs):
            mx = jnp.max(t, axis=1, keepdims=True)
            for k in range(t.shape[0] // 8):
                mk = jnp.broadcast_to(mx[8 * k:8 * k + 8], (8, b))
                for j in range((lo + 8 * k) // b, (hi + 8 * k) // b + 1):
                    accs[j] = jnp.where(diag == g0 + 8 * k - j * b, mk, accs[j])

        def empty(k):
            return [jnp.full((8, b), -jnp.inf, dt) for _ in range(k)]

        def fold(acc):
            return jnp.max(acc, axis=0, keepdims=True)

        def block_max(ref, r0):
            accs = empty(1)
            place(colmax(ref, r0, b), 0, 0, 0, accs)
            return fold(accs[0])

        def scoped(sems, ssems, rsems, reply, relay):
            e = nm + len(_TAIL)
            cps = [pltpu.make_async_copy(x_hbm.at[pl.ds(o, c)],
                                         buf.at[pl.ds(o - s0, c)], sems.at[i])
                   for i, (o, c) in enumerate(zip(offs, _MAIN))]
            cps[0].start()
            s_in = pltpu.make_async_copy(x_hbm.at[pl.ds(z0 + nx, ns)], sm, sems.at[e])
            s_in.start()
            s_out = pltpu.make_async_copy(sm, zs, sems.at[e + 1])

            cx, cy = lax.axis_index("x"), lax.axis_index("y")
            ynbr, xnbr, dnbr = (cx, 1 - cy), (1 - cx, cy), (1 - cx, 1 - cy)
            odd = (cx + cy) % 2 == 1
            succ = (jnp.where(odd, 1 - cx, cx), jnp.where(odd, cy, 1 - cy))
            pred = (jnp.where(odd, cx, 1 - cx), jnp.where(odd, 1 - cy, cy))
            bar = pltpu.get_barrier_semaphore()
            pl.semaphore_signal(bar, 1, device_id=succ, device_id_type=_MESH)

            own0 = pl.multiple_of(cy * b, b)
            oth0 = pl.multiple_of((1 - cy) * b, b)
            qk = pl.multiple_of(yq + cy * nq, 8)
            qo = pl.multiple_of(yq + (1 - cy) * nq, 8)
            zcps = [
                pltpu.make_async_copy(x_hbm.at[pl.ds(z0 + nx + ns, nzl)], zl,
                                      sems.at[e + 2]),
                pltpu.make_async_copy(x_hbm.at[pl.ds(pl.multiple_of(z0 + qk, 8), nq)],
                                      zq, sems.at[e + 3]),
            ]
            tcps = [pltpu.make_async_copy(
                        x_hbm.at[pl.ds(pl.multiple_of(own0 + o, 8), c)],
                        tbuf.at[pl.ds(o, c)], sems.at[nm + i])
                    for i, (o, c) in enumerate(zip(toffs, _TAIL))]
            for cp in zcps + cps[1:] + tcps:
                cp.start()

            sends = []

            def remote(src, dst, r, dev):
                rd = pltpu.make_async_remote_copy(
                    src, dst, ssems.at[len(sends)],
                    xb_sem if r is None else rsems.at[r],
                    device_id=dev, device_id_type=_MESH)
                sends.append(rd)
                return rd

            raw_q = remote(x_hbm.at[pl.ds(pl.multiple_of(z0 + qo, 8), nq)], rq, r_q, ynbr)
            raw_own = remote(x_hbm.at[pl.ds(oth0, b)], rown, r_own, ynbr)
            raw_x = remote(x_hbm.at[pl.ds(z0, nx)], rx, r_x, xnbr)

            pl.semaphore_wait(bar, 1)
            pl.semaphore_signal(reply, 1, device_id=pred, device_id_type=_MESH)

            @pl.when(odd)
            def _():
                raw_q.start()
                raw_own.start()
                pl.semaphore_wait(reply, 1)
                raw_x.start()

            @pl.when(jnp.logical_not(odd))
            def _():
                raw_x.start()
                pl.semaphore_wait(reply, 1)
                raw_q.start()
                raw_own.start()

            pl.semaphore_signal(relay, 1, device_id=succ, device_id_type=_MESH)

            sent = pz
            acc = None
            for i, (o, c) in enumerate(zip(offs, _MAIN)):
                cps[i].wait()
                if i == _BOUNCE_AT:
                    s_in.wait()
                    s_out.start()
                if i == _X_AT:
                    pl.semaphore_wait(relay, 1)
                    raw_x.wait_recv()
                    accs = empty(nxb)
                    place(colmax(rx, 0, nx), 0, 0, 0, accs)
                    for j in range(nxb):
                        hx[:, j * b:(j + 1) * b] = fold(accs[j])
                    remote(hx, xb, None, dnbr).start()
                    remote(hx, xa, r_xa, xnbr).start()

                nb = c // b
                u = max(d for d in range(1, _UNROLL + 1) if nb % d == 0)

                def blocks(k, carry, o=o, u=u):
                    for j in range(u):
                        r0 = pl.multiple_of(o - s0 + (k * u + j) * b, b)
                        part[:, pl.ds(pl.multiple_of(r0 + pz, b), b)] = block_max(buf, r0)
                    return carry

                if nb == u:
                    blocks(0, 0)
                else:
                    lax.fori_loop(0, nb // u, blocks, 0)
                if i in _SENDS:
                    done = o + c - p0
                    remote(part.at[:, pl.ds(sent, done - sent)],
                           recv.at[:, pl.ds(sent, done - sent)], r_part, ynbr).start()
                    sent = done
                if i == _ZONE_AT:
                    for cp in zcps:
                        cp.wait()
                    s_out.wait()
                    raw_q.wait_recv()
                    accs = empty(nzb)
                    place(jnp.maximum(colmax(zq, 0, nq), colmax(rq, 0, nq)),
                          qk, yq, yq + nq, accs)
                    place(colmax(zl, 0, nzl), nx + ns, nx + ns, nx + ns, accs)
                    place(colmax(zs, 0, ns), nx, nx, nx, accs)
                    for j in range(pb0, nzb):
                        part[:, (j - pb0) * b:(j - pb0 + 1) * b] = fold(accs[j])
                    remote(part.at[:, pl.ds(0, pz)], recv.at[:, pl.ds(0, pz)],
                           r_part, ynbr).start()
                if i == _OWN_AT:
                    raw_own.wait_recv()
                    acc = [jnp.broadcast_to(block_max(rown, 0), (8, b))]

            for i, (o, c) in enumerate(zip(toffs, _TAIL)):
                tcps[i].wait()
                place(colmax(tbuf, o, c), o, o, o, acc)
            o_ref[:, pl.ds(own0, b)] = fold(acc[0])
            remote(o_ref.at[:, pl.ds(own0, b)], o_ref.at[:, pl.ds(own0, b)],
                   r_fin, ynbr).start()

            pltpu.make_async_copy(xa, xa, rsems.at[r_xa]).wait()
            pltpu.make_async_copy(xb, xb, xb_sem).wait()
            pltpu.make_async_copy(recv, recv, rsems.at[r_part]).wait()
            ov = (nxb - pb0) * b
            if pb0:
                o_ref[:, z0:p0] = jnp.maximum(xa[:, :pb0 * b], xb[:, :pb0 * b])
            if ov:
                o_ref[:, p0:p0 + ov] = jnp.maximum(
                    jnp.maximum(xa[:, pb0 * b:], xb[:, pb0 * b:]),
                    jnp.maximum(part[:, :ov], recv[:, :ov]))
            o_ref[:, p0 + ov:] = jnp.maximum(part[:, ov:], recv[:, ov:])
            assert len(sends) == nsend
            for rd in sends:
                rd.wait_send()
            pltpu.make_async_copy(o_ref.at[:, pl.ds(oth0, b)],
                                  o_ref.at[:, pl.ds(oth0, b)], rsems.at[r_fin]).wait()

        pl.run_scoped(
            scoped,
            pltpu.SemaphoreType.DMA((nloc,)),
            pltpu.SemaphoreType.DMA((nsend,)),
            pltpu.SemaphoreType.DMA((6,)),
            pltpu.SemaphoreType.REGULAR,
            pltpu.SemaphoreType.REGULAR,
        )

    out = pl.pallas_call(
        body,
        out_shape=jax.ShapeDtypeStruct((1, m), dt),
        in_specs=[pl.BlockSpec(memory_space=pl.ANY)],
        out_specs=pl.BlockSpec(memory_space=pltpu.VMEM),
        scratch_shapes=[
            pltpu.VMEM((m - s0, n), dt),
            pltpu.VMEM((ns, n), dt),
            pltpu.VMEM((nzl, n), dt),
            pltpu.VMEM((nq, n), dt),
            pltpu.VMEM((b, n), dt),
            pltpu.VMEM((nq, n), dt),
            pltpu.VMEM((b, n), dt),
            pltpu.VMEM((nx, n), dt),
            pltpu.VMEM((1, m - p0), dt),
            pltpu.VMEM((1, m - p0), dt),
            pltpu.VMEM((1, nxb * b), dt),
            pltpu.VMEM((1, nxb * b), dt),
            pltpu.VMEM((1, nxb * b), dt),
            pltpu.SMEM((ns, n), dt),
            pltpu.SemaphoreType.DMA,
        ],
        compiler_params=pltpu.CompilerParams(
            vmem_limit_bytes=64 * 1024 * 1024, collective_id=0),
    )(x)
    return out.reshape(m, 1)
```

```python
import functools

import jax
import jax.numpy as jnp
from jax import lax
from jax.experimental import pallas as pl
from jax.experimental.pallas import tpu as pltpu

_MESH = pl.DeviceIdType.MESH
_B = 128
_U = 8
_NS = 10
_AHEAD = 8
_RAW_STEP = 6
_OWN_STEP = 42
_TAIL = (8, 8)
_TAIL_ORDER = (0, 8, 1, 9, 2, 10, 3, 11, 4, 12, 5, 13, 6, 14, 7, 15)


def pallas_dist_max_ax1_xy_m4096_n1024_kernel(x: jax.Array):
    m, n = x.shape
    dt = x.dtype
    b, u, ns = _B, _U, _NS
    s0 = 2 * b
    sr = (m - s0) // ns
    pb = sr // b
    spb = b // u
    steps = sr // u
    assert ns * pb * b == m - s0 and ns % 2 == 0 and n % 128 == 0
    assert sum(_TAIL) == spb and sorted(_TAIL_ORDER) == list(range(spb))
    toffs = [sum(_TAIL[:i]) for i in range(len(_TAIL))]
    last_issue = steps - _AHEAD
    nsend = pb + 2
    r_own, r_part, r_fin = range(3)

    def body(x_hbm, o_ref, buf, tbuf, rown, part, recv):
        diag = (lax.broadcasted_iota(jnp.int32, (u, b), 1)
                - lax.broadcasted_iota(jnp.int32, (u, b), 0))

        def row_max(ref, r0, rows):
            cols = [ref[pl.ds(r0, rows), j * 128:(j + 1) * 128]
                    for j in range(n // 128)]
            while len(cols) > 1:
                nxt = [jnp.maximum(cols[i], cols[i + 1])
                       for i in range(0, len(cols) - 1, 2)]
                cols = nxt + cols[2 * len(nxt):]
            mx = jnp.max(cols[0], axis=1, keepdims=True)
            return [jnp.broadcast_to(mx[u * k:u * (k + 1)], (u, b))
                    for k in range(rows // u)]

        def empty():
            return jnp.full((u, b), -jnp.inf, dt)

        def fold(acc):
            return jnp.max(acc, axis=0, keepdims=True)

        def scoped(sems, tsems, ssems, rsems):
            def issue(g):
                for s in range(ns):
                    r = s0 + s * sr + g * u
                    if not isinstance(r, int):
                        r = pl.multiple_of(r, u)
                    pltpu.make_async_copy(
                        x_hbm.at[pl.ds(r, u)], buf.at[g, pl.ds(s * u, u)],
                        sems.at[g]).start(priority=s % 2)

            issue(0)
            cy = lax.axis_index("y")
            nbr = (lax.axis_index("x"), 1 - cy)
            own0 = pl.multiple_of(cy * b, b)
            oth0 = pl.multiple_of((1 - cy) * b, b)
            bar = pltpu.get_barrier_semaphore()
            pl.semaphore_signal(bar, 1, device_id=nbr, device_id_type=_MESH)

            def prologue(g, carry):
                issue(g)
                return carry

            lax.fori_loop(1, _AHEAD, prologue, 0)

            sends = []

            def remote(src, dst, r):
                rd = pltpu.make_async_remote_copy(
                    src, dst, ssems.at[len(sends)], rsems.at[r],
                    device_id=nbr, device_id_type=_MESH)
                sends.append(rd)
                return rd

            raw = remote(x_hbm.at[pl.ds(oth0, b)], rown, r_own)

            def step(g, accs, do_issue):
                if do_issue:
                    issue(g + _AHEAD)
                pltpu.make_async_copy(buf.at[g], buf.at[g], sems.at[g]).wait()
                tiles = row_max(buf.at[g], 0, ns * u)
                mask = diag == (g % spb) * u
                return tuple(jnp.where(mask, t, a) for t, a in zip(tiles, accs))

            tacc = None
            for ph in range(pb):
                accs = tuple(empty() for _ in range(ns))
                lo0, hi0 = ph * spb, (ph + 1) * spb
                cuts = sorted({lo0, hi0} | {
                    c for c in (last_issue, _RAW_STEP, _OWN_STEP) if lo0 < c < hi0})
                for lo, hi in zip(cuts[:-1], cuts[1:]):
                    if lo == _RAW_STEP:
                        pl.semaphore_wait(bar, 1)
                        raw.start()
                    if lo == last_issue:
                        for p, (o, c) in enumerate(zip(toffs, _TAIL)):
                            for k in range(o, o + c):
                                r = pl.multiple_of(own0 + u * _TAIL_ORDER[k], u)
                                pltpu.make_async_copy(
                                    x_hbm.at[pl.ds(r, u)], tbuf.at[pl.ds(u * k, u)],
                                    tsems.at[p]).start(priority=k % 2)
                    if lo == _OWN_STEP:
                        raw.wait_recv()
                        acc = empty()
                        for k, t in enumerate(row_max(rown, 0, b)):
                            acc = jnp.where(diag == u * k, t, acc)
                        tacc = jnp.broadcast_to(fold(acc), (u, b))
                    accs = lax.fori_loop(
                        lo, hi, functools.partial(step, do_issue=lo < last_issue), accs)
                for s in range(ns):
                    part[:, (ph * ns + s) * b:(ph * ns + s + 1) * b] = fold(accs[s])
                sl = pl.ds(ph * ns * b, ns * b)
                remote(part.at[:, sl], recv.at[:, sl], r_part).start()

            for p, (o, c) in enumerate(zip(toffs, _TAIL)):
                sl = tbuf.at[pl.ds(u * o, u * c)]
                pltpu.make_async_copy(sl, sl, tsems.at[p]).wait()
                for k, t in enumerate(row_max(tbuf, u * o, u * c)):
                    tacc = jnp.where(diag == u * _TAIL_ORDER[o + k], t, tacc)
            o_ref[:, pl.ds(own0, b)] = fold(tacc)
            remote(o_ref.at[:, pl.ds(own0, b)], o_ref.at[:, pl.ds(own0, b)],
                   r_fin).start()

            pltpu.make_async_copy(recv, recv, rsems.at[r_part]).wait()
            for ph in range(pb):
                for s in range(ns):
                    sl = slice((ph * ns + s) * b, (ph * ns + s + 1) * b)
                    r = s0 + s * sr + ph * b
                    o_ref[:, r:r + b] = jnp.maximum(part[:, sl], recv[:, sl])
            assert len(sends) == nsend
            for rd in sends:
                rd.wait_send()
            pltpu.make_async_copy(o_ref.at[:, pl.ds(oth0, b)],
                                  o_ref.at[:, pl.ds(oth0, b)],
                                  rsems.at[r_fin]).wait()

        pl.run_scoped(
            scoped,
            pltpu.SemaphoreType.DMA((steps,)),
            pltpu.SemaphoreType.DMA((len(_TAIL),)),
            pltpu.SemaphoreType.DMA((nsend,)),
            pltpu.SemaphoreType.DMA((3,)),
        )

    out = pl.pallas_call(
        body,
        out_shape=jax.ShapeDtypeStruct((1, m), dt),
        in_specs=[pl.BlockSpec(memory_space=pl.ANY)],
        out_specs=pl.BlockSpec(memory_space=pltpu.VMEM),
        scratch_shapes=[
            pltpu.VMEM((steps, ns * u, n), dt),
            pltpu.VMEM((b, n), dt),
            pltpu.VMEM((b, n), dt),
            pltpu.VMEM((1, m - s0), dt),
            pltpu.VMEM((1, m - s0), dt),
        ],
        compiler_params=pltpu.CompilerParams(
            vmem_limit_bytes=64 * 1024 * 1024, collective_id=0),
    )(x)
    return out.reshape(m, 1)
```

```python
import functools

import jax
import jax.numpy as jnp
from jax import lax
from jax.experimental import pallas as pl
from jax.experimental.pallas import tpu as pltpu

_MESH = pl.DeviceIdType.MESH
_B = 128
_U = 8
_NS = 10
_AHEAD = 8
_LEAD = 4
_OTH_STEP = 6
_OWN_STEP = 32
_TAIL = (8, 8)
_TAIL_ORDER = (0, 8, 1, 9, 2, 10, 3, 11, 4, 12, 5, 13, 6, 14, 7, 15)


def pallas_dist_max_ax1_xy_m4096_n1024_kernel(x: jax.Array):
    m, n = x.shape
    dt = x.dtype
    b, u, ns = _B, _U, _NS
    s0 = 2 * b
    sr = (m - s0) // ns
    pb = sr // b
    spb = b // u
    steps = sr // u
    assert ns * pb * b == m - s0 and ns % 2 == 0 and n % 128 == 0
    assert sum(_TAIL) == spb and sorted(_TAIL_ORDER) == list(range(spb))
    toffs = [sum(_TAIL[:i]) for i in range(len(_TAIL))]
    last_issue = steps - _AHEAD
    nsend = pb + 2

    def body(x_hbm, o_ref, buf, tbuf, obuf, part, recv, opart, orecv):
        diag = (lax.broadcasted_iota(jnp.int32, (u, b), 1)
                - lax.broadcasted_iota(jnp.int32, (u, b), 0))

        def row_max(ref, r0, rows):
            cols = [ref[pl.ds(r0, rows), j * 128:(j + 1) * 128]
                    for j in range(n // 128)]
            while len(cols) > 1:
                nxt = [jnp.maximum(cols[i], cols[i + 1])
                       for i in range(0, len(cols) - 1, 2)]
                cols = nxt + cols[2 * len(nxt):]
            mx = jnp.max(cols[0], axis=1, keepdims=True)
            return [jnp.broadcast_to(mx[u * k:u * (k + 1)], (u, b))
                    for k in range(rows // u)]

        def empty():
            return jnp.full((u, b), -jnp.inf, dt)

        def fold(acc):
            return jnp.max(acc, axis=0, keepdims=True)

        def scoped(sems, tsems, osem, ssems, rsems):
            def fetch(r, dst, sem, priority):
                if not isinstance(r, int):
                    r = pl.multiple_of(r, u)
                pltpu.make_async_copy(
                    x_hbm.at[pl.ds(r, u)], dst, sem).start(priority=priority)

            def issue(g, streams=range(ns), priority=None):
                for s in streams:
                    fetch(s0 + s * sr + g * u, buf.at[g, pl.ds(s * u, u)], sems.at[g],
                          s % 2 if priority is None else priority)

            issue(0, range(_LEAD), 1)
            cy = lax.axis_index("y")
            nbr = (lax.axis_index("x"), 1 - cy)
            own0 = pl.multiple_of(cy * b, b)
            oth0 = pl.multiple_of((1 - cy) * b, b)
            for k in range(spb):
                fetch(oth0 + u * k, obuf.at[pl.ds(u * k, u)], osem, 1)
            issue(0, range(_LEAD, ns), 1)
            bar = pltpu.get_barrier_semaphore()
            pl.semaphore_signal(bar, 1, device_id=nbr, device_id_type=_MESH)

            def prologue(g, carry):
                issue(g)
                return carry

            lax.fori_loop(1, _AHEAD, prologue, 0)

            sends = []

            def remote(src, dst):
                k = len(sends)
                rd = pltpu.make_async_remote_copy(
                    src, dst, ssems.at[k], rsems.at[k],
                    device_id=nbr, device_id_type=_MESH)
                rd.start()
                sends.append(rd)

            def step(g, accs, do_issue):
                if do_issue:
                    issue(g + _AHEAD)
                pltpu.make_async_copy(buf.at[g], buf.at[g], sems.at[g]).wait()
                tiles = row_max(buf.at[g], 0, ns * u)
                mask = diag == (g % spb) * u
                return tuple(jnp.where(mask, t, a) for t, a in zip(tiles, accs))

            tacc = None
            for ph in range(pb):
                accs = tuple(empty() for _ in range(ns))
                lo0, hi0 = ph * spb, (ph + 1) * spb
                cuts = sorted({lo0, hi0} | {
                    c for c in (last_issue, _OTH_STEP, _OWN_STEP) if lo0 < c < hi0})
                for lo, hi in zip(cuts[:-1], cuts[1:]):
                    if lo == _OTH_STEP:
                        pltpu.make_async_copy(obuf, obuf, osem).wait()
                        acc = empty()
                        for k, t in enumerate(row_max(obuf, 0, b)):
                            acc = jnp.where(diag == u * k, t, acc)
                        opart[...] = fold(acc)
                        pl.semaphore_wait(bar, 1)
                        remote(opart, orecv)
                    if lo == last_issue:
                        for p, (o, c) in enumerate(zip(toffs, _TAIL)):
                            for k in range(o, o + c):
                                fetch(own0 + u * _TAIL_ORDER[k],
                                      tbuf.at[pl.ds(u * k, u)], tsems.at[p], k % 2)
                    if lo == _OWN_STEP:
                        sends[0].wait_recv()
                        tacc = jnp.broadcast_to(orecv[...], (u, b))
                    accs = lax.fori_loop(
                        lo, hi, functools.partial(step, do_issue=lo < last_issue), accs)
                for s in range(ns):
                    part[:, (ph * ns + s) * b:(ph * ns + s + 1) * b] = fold(accs[s])
                sl = pl.ds(ph * ns * b, ns * b)
                remote(part.at[:, sl], recv.at[:, sl])

            for p, (o, c) in enumerate(zip(toffs, _TAIL)):
                sl = tbuf.at[pl.ds(u * o, u * c)]
                pltpu.make_async_copy(sl, sl, tsems.at[p]).wait()
                for k, t in enumerate(row_max(tbuf, u * o, u * c)):
                    tacc = jnp.where(diag == u * _TAIL_ORDER[o + k], t, tacc)
            o_ref[:, pl.ds(own0, b)] = fold(tacc)
            remote(o_ref.at[:, pl.ds(own0, b)], o_ref.at[:, pl.ds(own0, b)])

            assert len(sends) == nsend
            for rd in sends:
                rd.wait_send()
            for ph in range(pb):
                sends[1 + ph].wait_recv()
                for s in range(ns):
                    sl = slice((ph * ns + s) * b, (ph * ns + s + 1) * b)
                    r = s0 + s * sr + ph * b
                    o_ref[:, r:r + b] = jnp.maximum(part[:, sl], recv[:, sl])
            pltpu.make_async_copy(o_ref.at[:, pl.ds(oth0, b)],
                                  o_ref.at[:, pl.ds(oth0, b)],
                                  rsems.at[nsend - 1]).wait()

        pl.run_scoped(
            scoped,
            pltpu.SemaphoreType.DMA((steps,)),
            pltpu.SemaphoreType.DMA((len(_TAIL),)),
            pltpu.SemaphoreType.DMA,
            pltpu.SemaphoreType.DMA((nsend,)),
            pltpu.SemaphoreType.DMA((nsend,)),
        )

    out = pl.pallas_call(
        body,
        out_shape=jax.ShapeDtypeStruct((1, m), dt),
        in_specs=[pl.BlockSpec(memory_space=pl.ANY)],
        out_specs=pl.BlockSpec(memory_space=pltpu.VMEM),
        scratch_shapes=[
            pltpu.VMEM((steps, ns * u, n), dt),
            pltpu.VMEM((b, n), dt),
            pltpu.VMEM((b, n), dt),
            pltpu.VMEM((1, m - s0), dt),
            pltpu.VMEM((1, m - s0), dt),
            pltpu.VMEM((1, b), dt),
            pltpu.VMEM((1, b), dt),
        ],
        compiler_params=pltpu.CompilerParams(
            vmem_limit_bytes=64 * 1024 * 1024, collective_id=0),
    )(x)
    return out.reshape(m, 1)
```

```python
import functools

import jax
import jax.numpy as jnp
from jax import lax
from jax.experimental import pallas as pl
from jax.experimental.pallas import tpu as pltpu

_MESH = pl.DeviceIdType.MESH
_B = 128
_H = 1
_NS = 10
_AHEAD = 8
_LEAD = 4
_OTH_STEP = 6
_OWN_STEP = 32
_TAIL = (0, 8, 16)


def pallas_dist_max_ax1_xy_m4096_n1024_kernel(x: jax.Array):
    m, n = x.shape
    dt = x.dtype
    b, h, ns = _B, _H, _NS
    c = n // 128
    ng = m // 8
    gpb = b // 8
    g0 = 2 * gpb
    steps = (ng - g0) // ns
    pb = steps // gpb
    assert n % 128 == 0 and ns * pb * gpb == ng - g0 and ns % 2 == 0 and 0 < h < c
    assert _TAIL[0] == 0 and _TAIL[-1] == gpb
    npc = len(_TAIL) - 1
    last_issue = steps - 1 - _AHEAD
    nsend = pb + 2

    def body(x_hbm, o_ref, buf, tbuf, obuf, part, recv, opart, orecv):
        diag = (lax.broadcasted_iota(jnp.int32, (8, b), 1)
                - lax.broadcasted_iota(jnp.int32, (8, b), 0))

        def row_max(tiles):
            while len(tiles) > 1:
                nxt = [jnp.maximum(tiles[i], tiles[i + 1])
                       for i in range(0, len(tiles) - 1, 2)]
                tiles = nxt + tiles[2 * len(nxt):]
            return jnp.broadcast_to(jnp.max(tiles[0], axis=1, keepdims=True), (8, b))

        def place(ref, groups, acc):
            for k in groups:
                t = row_max([ref[k * c + i] for i in range(c)])
                acc = jnp.where(diag == 8 * k, t, acc)
            return acc

        def empty():
            return jnp.full((8, b), -jnp.inf, dt)

        def fold(acc):
            return jnp.max(acc, axis=0, keepdims=True)

        def scoped(sems, tsems, osem, ssems, rsems):
            def fetch(t, nt, dst, sem, priority):
                pltpu.make_async_copy(
                    x_hbm.at[pl.ds(t, nt)], dst, sem).start(priority=priority)

            def issue(g, streams=range(ns), priority=None):
                for s in streams:
                    p = s % 2 if priority is None else priority
                    t = (g0 + s * steps + g) * c - h
                    if isinstance(g, int) and g == 0 and s == 0:
                        fetch(t + h, c - h, buf.at[0, pl.ds(h, c - h)], sems.at[0], p)
                        fetch(ng * c - h, h, buf.at[0, pl.ds(0, h)], sems.at[0], p)
                    else:
                        fetch(t, c, buf.at[g, pl.ds(s * c, c)], sems.at[g], p)

            def fetch_block(t0, dst, sem_of, priority_of):
                for j in range(gpb + 1):
                    lo, hi = max(c * j - h, 0), min(c * (j + 1) - h, gpb * c)
                    fetch(t0 + lo, hi - lo, dst.at[pl.ds(lo, hi - lo)],
                          sem_of(j), priority_of(j))

            issue(0, range(ns - 1, ns - 1 - _LEAD, -1), 1)
            cy = lax.axis_index("y")
            nbr = (lax.axis_index("x"), 1 - cy)
            own0 = pl.multiple_of(cy * b, b)
            oth0 = pl.multiple_of((1 - cy) * b, b)
            fetch_block((1 - cy) * (gpb * c), obuf, lambda j: osem, lambda j: 1)
            issue(0, range(ns - 1 - _LEAD, -1, -1), 1)
            bar = pltpu.get_barrier_semaphore()
            pl.semaphore_signal(bar, 1, device_id=nbr, device_id_type=_MESH)

            def prologue(g, carry):
                issue(g)
                return carry

            lax.fori_loop(1, _AHEAD + 1, prologue, 0)

            sends = []

            def remote(src, dst):
                k = len(sends)
                rd = pltpu.make_async_remote_copy(
                    src, dst, ssems.at[k], rsems.at[k],
                    device_id=nbr, device_id_type=_MESH)
                rd.start()
                sends.append(rd)

            def wait(g):
                pltpu.make_async_copy(buf.at[g], buf.at[g], sems.at[g]).wait()

            def reduce(j, accs, last=False):
                mask = diag == (j % gpb) * 8
                out = []
                for s in range(ns):
                    tiles = [buf[j, s * c + i] for i in range(h, c)]
                    if last:
                        tiles += [buf[0, (s + 1) % ns * c + i] for i in range(h)]
                    else:
                        tiles += [buf[j + 1, s * c + i] for i in range(h)]
                    out.append(jnp.where(mask, row_max(tiles), accs[s]))
                return tuple(out)

            def step(j, accs, do_issue):
                if do_issue:
                    issue(j + 1 + _AHEAD)
                wait(j + 1)
                return reduce(j, accs)

            wait(0)
            tacc = None
            for ph in range(pb):
                accs = tuple(empty() for _ in range(ns))
                lo0, hi0 = ph * gpb, min((ph + 1) * gpb, steps - 2)
                cuts = sorted({lo0, hi0} | {
                    e for e in (last_issue, _OTH_STEP, _OWN_STEP) if lo0 < e < hi0})
                for lo, hi in zip(cuts[:-1], cuts[1:]):
                    if lo == _OTH_STEP:
                        pltpu.make_async_copy(obuf, obuf, osem).wait()
                        opart[...] = fold(place(obuf, range(gpb), empty()))
                        pl.semaphore_wait(bar, 1)
                        remote(opart, orecv)
                    if lo == last_issue:
                        fetch_block(
                            cy * (gpb * c), tbuf,
                            lambda j: tsems.at[
                                min(p for p in range(npc) if j <= _TAIL[p + 1])],
                            lambda j: min(j, gpb - 1) % 2)
                    if lo == _OWN_STEP:
                        sends[0].wait_recv()
                        tacc = jnp.broadcast_to(orecv[...], (8, b))
                    accs = lax.fori_loop(
                        lo, hi, functools.partial(step, do_issue=lo < last_issue), accs)
                if ph == pb - 1:
                    wait(steps - 1)
                    accs = reduce(steps - 1, reduce(steps - 2, accs), last=True)
                for s in range(ns):
                    part[:, (ph * ns + s) * b:(ph * ns + s + 1) * b] = fold(accs[s])
                sl = pl.ds(ph * ns * b, ns * b)
                remote(part.at[:, sl], recv.at[:, sl])

            for p in range(npc):
                lo = c * (_TAIL[p] + 1) - h if p else 0
                hi = min(c * (_TAIL[p + 1] + 1) - h, gpb * c)
                sl = tbuf.at[pl.ds(lo, hi - lo)]
                pltpu.make_async_copy(sl, sl, tsems.at[p]).wait()
                tacc = place(tbuf, range(_TAIL[p], _TAIL[p + 1]), tacc)
            o_ref[:, pl.ds(own0, b)] = fold(tacc)
            remote(o_ref.at[:, pl.ds(own0, b)], o_ref.at[:, pl.ds(own0, b)])

            assert len(sends) == nsend
            for rd in sends:
                rd.wait_send()
            for ph in range(pb):
                sends[1 + ph].wait_recv()
                for s in range(ns):
                    sl = slice((ph * ns + s) * b, (ph * ns + s + 1) * b)
                    r = (g0 + s * steps) * 8 + ph * b
                    o_ref[:, r:r + b] = jnp.maximum(part[:, sl], recv[:, sl])
            pltpu.make_async_copy(o_ref.at[:, pl.ds(oth0, b)],
                                  o_ref.at[:, pl.ds(oth0, b)],
                                  rsems.at[nsend - 1]).wait()

        pl.run_scoped(
            scoped,
            pltpu.SemaphoreType.DMA((steps,)),
            pltpu.SemaphoreType.DMA((npc,)),
            pltpu.SemaphoreType.DMA,
            pltpu.SemaphoreType.DMA((nsend,)),
            pltpu.SemaphoreType.DMA((nsend,)),
        )

    tiles = x.reshape(ng, 8, c, 128).transpose(0, 2, 1, 3).reshape(ng * c, 8, 128)
    out = pl.pallas_call(
        body,
        out_shape=jax.ShapeDtypeStruct((1, m), dt),
        in_specs=[pl.BlockSpec(memory_space=pl.ANY)],
        out_specs=pl.BlockSpec(memory_space=pltpu.VMEM),
        scratch_shapes=[
            pltpu.VMEM((steps, ns * c, 8, 128), dt),
            pltpu.VMEM((gpb * c, 8, 128), dt),
            pltpu.VMEM((gpb * c, 8, 128), dt),
            pltpu.VMEM((1, m - 2 * b), dt),
            pltpu.VMEM((1, m - 2 * b), dt),
            pltpu.VMEM((1, b), dt),
            pltpu.VMEM((1, b), dt),
        ],
        compiler_params=pltpu.CompilerParams(
            vmem_limit_bytes=64 * 1024 * 1024, collective_id=0),
    )(tiles)
    return out.reshape(m, 1)
```

```python
import functools

import jax
import jax.numpy as jnp
from jax import lax
from jax.experimental import pallas as pl
from jax.experimental.pallas import tpu as pltpu

_MESH = pl.DeviceIdType.MESH
_B = 128
_H = 1
_NS = 10
_AHEAD = 8
_LEAD = 4
_OTH_STEP = 6
_OWN_STEP = 32
_TAIL = (0, 8, 16)


def pallas_dist_max_ax1_xy_m4096_n1024_kernel(x: jax.Array):
    m, n = x.shape
    dt = x.dtype
    b, h, ns = _B, _H, _NS
    c = n // 128
    ng = m // 8
    gpb = b // 8
    g0 = 2 * gpb
    steps = (ng - g0) // ns
    pb = steps // gpb
    assert n % 128 == 0 and ns * pb * gpb == ng - g0 and ns % 2 == 0 and 0 < h < c
    assert _TAIL[0] == 0 and _TAIL[-1] == gpb
    npc = len(_TAIL) - 1
    last_issue = steps - 1 - _AHEAD
    nsend = pb + 2

    def body(x_hbm, o_ref, buf, tbuf, obuf, part, recv, opart, orecv):
        diag = (lax.broadcasted_iota(jnp.int32, (8, b), 1)
                - lax.broadcasted_iota(jnp.int32, (8, b), 0))

        def row_max(*slabs):
            ts = [v[:, i] for v in slabs for i in range(v.shape[1])]
            while len(ts) > 1:
                nxt = [jnp.maximum(ts[i], ts[i + 1]) for i in range(0, len(ts) - 1, 2)]
                ts = nxt + ts[2 * len(nxt):]
            return jnp.broadcast_to(jnp.max(ts[0], axis=2, keepdims=True),
                                    ts[0].shape[:2] + (b,))

        def place(ref, lo, hi, acc):
            t = row_max(ref[lo * c:hi * c].reshape(hi - lo, c, 8, 128))
            for k in range(lo, hi):
                acc = jnp.where(diag == 8 * k, t[k - lo], acc)
            return acc

        def scoped(sems, tsems, osem, ssems, rsems):
            def fetch(t, nt, dst, sem, priority):
                pltpu.make_async_copy(
                    x_hbm.at[pl.ds(t, nt)], dst, sem).start(priority=priority)

            def issue(g, streams=range(ns), priority=None):
                for s in streams:
                    p = s % 2 if priority is None else priority
                    t = (g0 + s * steps + g) * c - h
                    if isinstance(g, int) and g == 0 and s == 0:
                        fetch(t + h, c - h, buf.at[0, 0, pl.ds(h, c - h)], sems.at[0], p)
                        fetch(ng * c - h, h, buf.at[0, 0, pl.ds(0, h)], sems.at[0], p)
                    else:
                        fetch(t, c, buf.at[g, s], sems.at[g], p)

            def fetch_block(t0, dst, sem_of, priority_of):
                for j in range(gpb + 1):
                    lo, hi = max(c * j - h, 0), min(c * (j + 1) - h, gpb * c)
                    fetch(t0 + lo, hi - lo, dst.at[pl.ds(lo, hi - lo)],
                          sem_of(j), priority_of(j))

            issue(0, range(ns - 1, ns - 1 - _LEAD, -1), 1)
            cy = lax.axis_index("y")
            nbr = (lax.axis_index("x"), 1 - cy)
            fetch_block((1 - cy) * (gpb * c), obuf, lambda j: osem, lambda j: 1)
            issue(0, range(ns - 1 - _LEAD, -1, -1), 1)
            bar = pltpu.get_barrier_semaphore()
            pl.semaphore_signal(bar, 1, device_id=nbr, device_id_type=_MESH)

            def prologue(g, carry):
                issue(g)
                return carry

            lax.fori_loop(1, _AHEAD + 1, prologue, 0)

            sends = []

            def remote(src, dst):
                k = len(sends)
                rd = pltpu.make_async_remote_copy(
                    src, dst, ssems.at[k], rsems.at[k],
                    device_id=nbr, device_id_type=_MESH)
                rd.start()
                sends.append(rd)

            def wait(g):
                pltpu.make_async_copy(buf.at[g], buf.at[g], sems.at[g]).wait()

            def reduce(j, acc, rest):
                t = row_max(buf[j, :, h:c], rest)
                return jnp.where((diag == (j % gpb) * 8)[None], t, acc)

            def step(j, acc, do_issue):
                if do_issue:
                    issue(j + 1 + _AHEAD)
                wait(j + 1)
                return reduce(j, acc, buf[j + 1, :, 0:h])

            wait(0)
            tacc = None
            for ph in range(pb):
                acc = jnp.full((ns, 8, b), -jnp.inf, dt)
                lo0, hi0 = ph * gpb, min((ph + 1) * gpb, steps - 2)
                cuts = sorted({lo0, hi0} | {
                    e for e in (last_issue, _OTH_STEP, _OWN_STEP) if lo0 < e < hi0})
                for lo, hi in zip(cuts[:-1], cuts[1:]):
                    if lo == _OTH_STEP:
                        pltpu.make_async_copy(obuf, obuf, osem).wait()
                        opart[...] = jnp.max(
                            place(obuf, 0, gpb, jnp.full((8, b), -jnp.inf, dt)),
                            axis=0, keepdims=True)
                        pl.semaphore_wait(bar, 1)
                        remote(opart, orecv)
                    if lo == last_issue:
                        fetch_block(
                            cy * (gpb * c), tbuf,
                            lambda j: tsems.at[
                                min(p for p in range(npc) if j <= _TAIL[p + 1])],
                            lambda j: min(j, gpb - 1) % 2)
                    if lo == _OWN_STEP:
                        sends[0].wait_recv()
                        tacc = jnp.broadcast_to(orecv[...], (8, b))
                    acc = lax.fori_loop(
                        lo, hi, functools.partial(step, do_issue=lo < last_issue), acc)
                if ph == pb - 1:
                    acc = step(steps - 2, acc, False)
                    wrap = jnp.concatenate([buf[0, 1:ns, 0:h], buf[0, 0:1, 0:h]], axis=0)
                    acc = reduce(steps - 1, acc, wrap)
                part[ph] = jnp.max(acc, axis=1, keepdims=True)
                remote(part.at[ph], recv.at[ph])

            for p in range(npc):
                lo = c * (_TAIL[p] + 1) - h if p else 0
                hi = min(c * (_TAIL[p + 1] + 1) - h, gpb * c)
                sl = tbuf.at[pl.ds(lo, hi - lo)]
                pltpu.make_async_copy(sl, sl, tsems.at[p]).wait()
                tacc = place(tbuf, _TAIL[p], _TAIL[p + 1], tacc)
            o_ref[cy] = jnp.max(tacc, axis=0, keepdims=True)
            remote(o_ref.at[cy], o_ref.at[cy])

            assert len(sends) == nsend
            for rd in sends:
                rd.wait_send()
            for ph in range(pb):
                sends[1 + ph].wait_recv()
                res = jnp.maximum(part[ph], recv[ph])
                for s in range(ns):
                    o_ref[2 + s * pb + ph] = res[s]
            pltpu.make_async_copy(o_ref.at[1 - cy], o_ref.at[1 - cy],
                                  rsems.at[nsend - 1]).wait()

        pl.run_scoped(
            scoped,
            pltpu.SemaphoreType.DMA((steps,)),
            pltpu.SemaphoreType.DMA((npc,)),
            pltpu.SemaphoreType.DMA,
            pltpu.SemaphoreType.DMA((nsend,)),
            pltpu.SemaphoreType.DMA((nsend,)),
        )

    tiles = x.reshape(ng, 8, c, 128).transpose(0, 2, 1, 3).reshape(ng * c, 8, 128)
    out = pl.pallas_call(
        body,
        out_shape=jax.ShapeDtypeStruct((m // b, 1, b), dt),
        in_specs=[pl.BlockSpec(memory_space=pl.ANY)],
        out_specs=pl.BlockSpec(memory_space=pltpu.VMEM),
        scratch_shapes=[
            pltpu.VMEM((steps, ns, c, 8, 128), dt),
            pltpu.VMEM((gpb * c, 8, 128), dt),
            pltpu.VMEM((gpb * c, 8, 128), dt),
            pltpu.VMEM((pb, ns, 1, b), dt),
            pltpu.VMEM((pb, ns, 1, b), dt),
            pltpu.VMEM((1, b), dt),
            pltpu.VMEM((1, b), dt),
        ],
        compiler_params=pltpu.CompilerParams(
            vmem_limit_bytes=64 * 1024 * 1024, collective_id=0),
    )(tiles)
    return out.reshape(m, 1)
```
